```python
import numpy as np

kernel_name = "dist_rope_attn_htp_bs_b2_sq512_d1024_hq8_dh128"

def setup_inputs():
    x = np.random.randn(8, 512, 1024).astype(np.float32)
    Wq = np.random.randn(1024, 4096).astype(np.float32) * 0.02
    Wk = np.random.randn(1024, 4096).astype(np.float32) * 0.02
    Wv = np.random.randn(1024, 4096).astype(np.float32) * 0.02
    Wo = np.random.randn(4096, 1024).astype(np.float32) * 0.02
    return {"x": x, "Wq": Wq, "Wk": Wk, "Wv": Wv, "Wo": Wo}

def reference(x, Wq, Wk, Wv, Wo):
    B, Sq, Hq, Dh = 8, 512, 32, 128
    inv = 1.0 / (10000.0 ** (np.arange(0, Dh, 2) / Dh))
    pos = np.arange(Sq)[:, None] * inv[None, :]
    cos = np.repeat(np.cos(pos), 2, axis=-1).astype(np.float32)
    sin = np.repeat(np.sin(pos), 2, axis=-1).astype(np.float32)
    def rot(t):
        t2 = t.reshape(B, Sq, Hq, Dh // 2, 2)
        t_r = np.stack([-t2[..., 1], t2[..., 0]], axis=-1).reshape(B, Sq, Hq, Dh)
        return t * cos[None, :, None, :] + t_r * sin[None, :, None, :]
    Q = rot((x @ Wq).reshape(B, Sq, Hq, Dh))
    K = rot((x @ Wk).reshape(B, Sq, Hq, Dh))
    V = (x @ Wv).reshape(B, Sq, Hq, Dh)
    s = np.einsum('bihd,bjhd->bhij', Q, K).astype(np.float32) * 0.08838834764831843
    s_max = s.max(axis=-1, keepdims=True)
    w = np.exp(s - s_max)
    w = w / w.sum(axis=-1, keepdims=True)
    ctx = np.einsum('bhij,bjhd->bihd', w, V).reshape(B, Sq, Hq * Dh)
    return ctx @ Wo
```

```python
import jax
import jax.numpy as jnp
import numpy as np
from jax import lax
from jax.experimental import pallas as pl
from jax.experimental.pallas import tpu as pltpu

N_DEV = 4
BL, S, D = 2, 512, 1024
HL, DH = 8, 128
SCALE = 0.08838834764831843
LOG2E = 1.4426950408889634


def _rope_tables():
    inv = 1.0 / (10000.0 ** (np.arange(0, DH, 2) / DH))
    pos = np.arange(S)[:, None] * inv[None, :]
    cos = np.repeat(np.cos(pos), 2, axis=-1).astype(np.float32)
    sin = np.repeat(np.sin(pos), 2, axis=-1).astype(np.float32)
    sign = np.where(np.arange(DH) % 2 == 0, -1.0, 1.0).astype(np.float32)
    sin = sin * sign[None, :]
    c = np.float32(SCALE * LOG2E)
    return np.stack([cos * c, sin * c, cos, sin]).astype(np.float32)


_TABLES = _rope_tables()


def pallas_dist_rope_attn_htp_bs_b2_sq512_d1024_hq8_dh128_kernel(x, Wq, Wk, Wv, Wo):
    f32, bf16 = jnp.float32, jnp.bfloat16
    MESH = pl.DeviceIdType.MESH

    def body(x_hbm, wq_hbm, wk_hbm, wv_hbm, wo_hbm, tab_ref, out_hbm,
             xst, wst, wb, x_all, ctx, own0, sbuf, rbuf, ost,
             ld_sems, ag_s, ag_r, rs_s, rs_r, out_sems):
        me = lax.axis_index("i")
        right = lax.rem(me + 1, N_DEV)
        left = lax.rem(me + 3, N_DEV)
        diag = lax.rem(me + 2, N_DEV)

        x_ld = [pltpu.make_async_copy(x_hbm.at[b], xst.at[b], ld_sems.at[b]) for b in range(BL)]
        w_ld = [pltpu.make_async_copy(w, wst.at[i], ld_sems.at[2 + i])
                for i, w in enumerate((wq_hbm, wk_hbm, wv_hbm, wo_hbm))]
        x_ld[0].start()
        x_ld[1].start()
        for c in w_ld:
            c.start()

        def ag(src_slot, dst_slot, dev):
            return pltpu.make_async_remote_copy(
                src_ref=x_all.at[src_slot], dst_ref=x_all.at[dst_slot],
                send_sem=ag_s.at[dst_slot - 1], recv_sem=ag_r.at[dst_slot - 1],
                device_id=(dev,), device_id_type=MESH)

        x_ld[0].wait()
        x_all[0] = xst[0].astype(bf16)
        ag(0, 1, left).start()
        ag(0, 2, right).start()
        ag(0, 3, diag).start()
        x_ld[1].wait()
        x_all[7] = xst[1].astype(bf16)
        ag(7, 4, diag).start()
        ag(7, 5, left).start()
        ag(7, 6, right).start()
        for i in range(4):
            w_ld[i].wait()
            wb[i] = wst[i].astype(bf16)

        even = (lax.broadcasted_iota(jnp.int32, (S, DH), 1) % 2) == 0

        def rope(t, c, s):
            sw = jnp.where(even, pltpu.roll(t, DH - 1, 1), pltpu.roll(t, 1, 1))
            return (t * c + sw * s).astype(bf16)

        def rs(step, dev):
            return pltpu.make_async_remote_copy(
                src_ref=sbuf.at[step - 1], dst_ref=rbuf.at[step - 1],
                send_sem=rs_s.at[step - 1], recv_sem=rs_r.at[step - 1],
                device_id=(dev,), device_id_type=MESH)

        def step_fn(s, carry):
            @pl.when(jnp.logical_and(s >= 1, s <= 6))
            def _():
                ag(0, s, me).wait_recv()

            xb = x_all[s]
            for hp in range(HL // 2):
                cols = slice(hp * 2 * DH, (hp + 1) * 2 * DH)
                q2 = jnp.dot(xb, wb[0, :, cols], preferred_element_type=f32)
                k2 = jnp.dot(xb, wb[1, :, cols], preferred_element_type=f32)
                v2 = jnp.dot(xb, wb[2, :, cols], preferred_element_type=f32).astype(bf16)
                for j in range(2):
                    h = hp * 2 + j
                    hs = slice(j * DH, (j + 1) * DH)
                    q = rope(q2[:, hs], tab_ref[0], tab_ref[1])
                    k = rope(k2[:, hs], tab_ref[2], tab_ref[3])
                    sc = lax.dot_general(q, k, (((1,), (1,)), ((), ())),
                                         preferred_element_type=f32)
                    m = jnp.max(sc, axis=-1, keepdims=True)
                    p = jnp.exp2(sc - m)
                    l = jnp.sum(p, axis=-1, keepdims=True)
                    o = jnp.dot(p.astype(bf16), v2[:, hs], preferred_element_type=f32)
                    ctx[:, h * DH:(h + 1) * DH] = (o / l).astype(bf16)
            part = jnp.dot(ctx[...], wb[3], preferred_element_type=f32)

            @pl.when(s == 0)
            def _():
                own0[...] = part

            @pl.when(jnp.logical_and(s >= 1, s <= 6))
            def _():
                sbuf[s - 1] = part.astype(bf16)
                off = jnp.where(jnp.logical_or(s == 1, s == 5), 1,
                                jnp.where(jnp.logical_or(s == 2, s == 6), 3, 2))
                rs(s, lax.rem(me + off, N_DEV)).start()

            @pl.when(s == 6)
            def _():
                for t in (1, 2, 3):
                    rs(t, me).wait_recv()
                ost[0] = (own0[...] + rbuf[0].astype(f32)) + (rbuf[1].astype(f32) + rbuf[2].astype(f32))
                pltpu.make_async_copy(ost.at[0], out_hbm.at[0], out_sems.at[0]).start()

            @pl.when(s == 7)
            def _():
                for t in (4, 5, 6):
                    rs(t, me).wait_recv()
                ost[1] = (part + rbuf[3].astype(f32)) + (rbuf[4].astype(f32) + rbuf[5].astype(f32))
                pltpu.make_async_copy(ost.at[1], out_hbm.at[1], out_sems.at[1]).start()
            return carry

        lax.fori_loop(0, 8, step_fn, 0)

        for t in range(1, 7):
            ag(0, t, me).wait_send()
            rs(t, me).wait_send()
        for b in range(BL):
            pltpu.make_async_copy(ost.at[b], out_hbm.at[b], out_sems.at[b]).wait()

    any_spec = pl.BlockSpec(memory_space=pl.ANY)
    return pl.pallas_call(
        body,
        out_shape=jax.ShapeDtypeStruct((BL, S, D), f32),
        in_specs=[any_spec] * 5 + [pl.BlockSpec(memory_space=pltpu.VMEM)],
        out_specs=any_spec,
        scratch_shapes=[
            pltpu.VMEM((BL, S, D), f32),
            pltpu.VMEM((4, D, D), f32),
            pltpu.VMEM((4, D, D), bf16),
            pltpu.VMEM((8, S, D), bf16),
            pltpu.VMEM((S, D), bf16),
            pltpu.VMEM((S, D), f32),
            pltpu.VMEM((6, S, D), bf16),
            pltpu.VMEM((6, S, D), bf16),
            pltpu.VMEM((BL, S, D), f32),
            pltpu.SemaphoreType.DMA((6,)),
            pltpu.SemaphoreType.DMA((6,)),
            pltpu.SemaphoreType.DMA((6,)),
            pltpu.SemaphoreType.DMA((6,)),
            pltpu.SemaphoreType.DMA((6,)),
            pltpu.SemaphoreType.DMA((2,)),
        ],
        compiler_params=pltpu.CompilerParams(vmem_limit_bytes=100 * 1024 * 1024),
    )(x, Wq, Wk, Wv, Wo, jnp.asarray(_TABLES))
```

```python
import jax
import jax.numpy as jnp
import numpy as np
from jax import lax
from jax.experimental import pallas as pl
from jax.experimental.pallas import tpu as pltpu

N_DEV = 4
BL, S, D = 2, 512, 1024
HL, DH = 8, 128
NT = 4
SCALE = 0.08838834764831843
LOG2E = 1.4426950408889634


def _rope_tables():
    inv = 1.0 / (10000.0 ** (np.arange(0, DH, 2) / DH))
    pos = np.arange(S)[:, None] * inv[None, :]
    cos = np.repeat(np.cos(pos), 2, axis=-1).astype(np.float32)
    sin = np.repeat(np.sin(pos), 2, axis=-1).astype(np.float32)
    sign = np.where(np.arange(DH) % 2 == 0, -1.0, 1.0).astype(np.float32)
    sin = sin * sign[None, :]
    c = np.float32(SCALE * LOG2E)
    return np.stack([cos * c, sin * c, cos, sin]).astype(np.float32)


_TABLES = _rope_tables()


def pallas_dist_rope_attn_htp_bs_b2_sq512_d1024_hq8_dh128_kernel(x, Wq, Wk, Wv, Wo):
    f32, bf16 = jnp.float32, jnp.bfloat16
    MESH = pl.DeviceIdType.MESH

    def body(x_hbm, wq_hbm, wk_hbm, wv_hbm, wo_hbm, tab_ref, out_hbm,
             xst, wst, wb, x_all, ctx, own0, sbuf, rbuf, ost,
             x_sems, w_sems, ag_s, ag_r, rs_s, rs_r, out_sems):
        me = lax.axis_index("i")
        right = lax.rem(me + 1, N_DEV)
        left = lax.rem(me + 3, N_DEV)
        diag = lax.rem(me + 2, N_DEV)

        NP = HL // 2
        PW = 2 * DH
        w_hbm = (wq_hbm, wk_hbm, wv_hbm)

        def x_ld(b):
            return pltpu.make_async_copy(x_hbm.at[b], xst.at[b], x_sems.at[b])

        def w_ld(i, hp):
            cols = pl.ds(hp * PW, PW)
            return pltpu.make_async_copy(w_hbm[i].at[:, cols], wst.at[i, :, cols],
                                         w_sems.at[i * NP + hp])

        wo_ld = pltpu.make_async_copy(wo_hbm, wst.at[3], w_sems.at[3 * NP])

        def ag(src_slot, dst_slot, dev):
            return pltpu.make_async_remote_copy(
                src_ref=x_all.at[src_slot], dst_ref=x_all.at[dst_slot],
                send_sem=ag_s.at[dst_slot - 1], recv_sem=ag_r.at[dst_slot - 1],
                device_id=(dev,), device_id_type=MESH)

        def rs(step, dev):
            return pltpu.make_async_remote_copy(
                src_ref=sbuf.at[step - 1], dst_ref=rbuf.at[step - 1],
                send_sem=rs_s.at[step - 1], recv_sem=rs_r.at[step - 1],
                device_id=(dev,), device_id_type=MESH)

        even = (lax.broadcasted_iota(jnp.int32, (S, DH), 1) % 2) == 0

        def rope(t, c, s):
            sw = jnp.where(even, pltpu.roll(t, DH - 1, 1), pltpu.roll(t, 1, 1))
            return (t * c + sw * s).astype(bf16)

        def attention(slot, first=False):
            xb = x_all[slot]
            for hp in range(NP):
                cols = slice(hp * PW, (hp + 1) * PW)
                qkv = []
                for i in range(3):
                    if first:
                        w_ld(i, hp).wait()
                        nxt = hp * 3 + i + 2
                        if nxt < 3 * NP:
                            w_ld(nxt % 3, nxt // 3).start()
                        elif nxt == 3 * NP:
                            wo_ld.start()
                        else:
                            x_ld(1).start()
                        wb[i, :, cols] = wst[i, :, cols].astype(bf16)
                    qkv.append(jnp.dot(xb, wb[i, :, cols], preferred_element_type=f32))
                if first and hp == 1:
                    ag(0, 3, diag).start()
                q2, k2, v2 = qkv[0], qkv[1], qkv[2].astype(bf16)
                for j in range(2):
                    h = hp * 2 + j
                    hs = slice(j * DH, (j + 1) * DH)
                    q = rope(q2[:, hs], tab_ref[0], tab_ref[1])
                    k = rope(k2[:, hs], tab_ref[2], tab_ref[3])
                    sc = lax.dot_general(q, k, (((1,), (1,)), ((), ())),
                                         preferred_element_type=f32)
                    m = jnp.max(sc, axis=-1, keepdims=True)
                    p = jnp.exp2(sc - m)
                    l = jnp.sum(p, axis=-1, keepdims=True)
                    o = jnp.dot(p.astype(bf16), v2[:, hs], preferred_element_type=f32)
                    ctx[:, h * DH:(h + 1) * DH] = (o / l).astype(bf16)

        x_ld(0).start()
        w_ld(0, 0).start()
        w_ld(1, 0).start()
        x_ld(0).wait()
        x_all[0] = xst[0].astype(bf16)
        ag(0, 1, left).start()
        ag(0, 2, right).start()
        attention(0, first=True)
        wo_ld.wait()
        wb[3] = wst[3].astype(bf16)
        own0[...] = jnp.dot(ctx[...], wb[3], preferred_element_type=f32)
        x_ld(1).wait()
        x_all[7] = xst[1].astype(bf16)
        ag(7, 4, diag).start()
        ag(7, 5, left).start()
        ag(7, 6, right).start()

        def step_fn(s, carry):
            ag(0, s, me).wait_recv()
            attention(s)
            part = jnp.dot(ctx[...], wb[3], preferred_element_type=f32)
            sbuf[s - 1] = part.astype(bf16)
            off = jnp.where(jnp.logical_or(s == 1, s == 5), 1,
                            jnp.where(jnp.logical_or(s == 2, s == 6), 3, 2))
            rs(s, lax.rem(me + off, N_DEV)).start()
            return carry

        lax.fori_loop(1, 7, step_fn, 0)

        for t in (1, 2, 3):
            rs(t, me).wait_recv()
        ost[0] = (own0[...] + rbuf[0].astype(f32)) + (rbuf[1].astype(f32) + rbuf[2].astype(f32))
        out0 = pltpu.make_async_copy(ost.at[0], out_hbm.at[0], out_sems.at[0])
        out0.start()
        attention(7)
        for t in (4, 5, 6):
            rs(t, me).wait_recv()
        outs = []
        for c in range(NT):
            cs = pl.ds(c * (D // NT), D // NT)
            part = jnp.dot(ctx[...], wb[3, :, cs], preferred_element_type=f32)
            ost[1, :, cs] = (part + rbuf[3, :, cs].astype(f32)) + (
                rbuf[4, :, cs].astype(f32) + rbuf[5, :, cs].astype(f32))
            cp = pltpu.make_async_copy(ost.at[1, :, cs], out_hbm.at[1, :, cs], out_sems.at[1 + c])
            cp.start()
            outs.append(cp)

        for t in range(1, 7):
            ag(0, t, me).wait_send()
            rs(t, me).wait_send()
        out0.wait()
        for cp in outs:
            cp.wait()

    any_spec = pl.BlockSpec(memory_space=pl.ANY)
    return pl.pallas_call(
        body,
        out_shape=jax.ShapeDtypeStruct((BL, S, D), f32),
        in_specs=[any_spec] * 5 + [pl.BlockSpec(memory_space=pltpu.VMEM)],
        out_specs=any_spec,
        scratch_shapes=[
            pltpu.VMEM((BL, S, D), f32),
            pltpu.VMEM((4, D, D), f32),
            pltpu.VMEM((4, D, D), bf16),
            pltpu.VMEM((8, S, D), bf16),
            pltpu.VMEM((S, D), bf16),
            pltpu.VMEM((S, D), f32),
            pltpu.VMEM((6, S, D), bf16),
            pltpu.VMEM((6, S, D), bf16),
            pltpu.VMEM((BL, S, D), f32),
            pltpu.SemaphoreType.DMA((2,)),
            pltpu.SemaphoreType.DMA((13,)),
            pltpu.SemaphoreType.DMA((6,)),
            pltpu.SemaphoreType.DMA((6,)),
            pltpu.SemaphoreType.DMA((6,)),
            pltpu.SemaphoreType.DMA((6,)),
            pltpu.SemaphoreType.DMA((1 + NT,)),
        ],
        compiler_params=pltpu.CompilerParams(vmem_limit_bytes=100 * 1024 * 1024),
    )(x, Wq, Wk, Wv, Wo, jnp.asarray(_TABLES))
```

```python
import jax
import jax.numpy as jnp
import numpy as np
from jax import lax
from jax.experimental import pallas as pl
from jax.experimental.pallas import tpu as pltpu

N_DEV = 4
BL, S, D = 2, 512, 1024
HL, DH = 8, 128
SCALE = 0.08838834764831843
LOG2E = 1.4426950408889634


def _rope_tables():
    inv = 1.0 / (10000.0 ** (np.arange(0, DH, 2) / DH))
    pos = np.arange(S)[:, None] * inv[None, :]
    cos = np.repeat(np.cos(pos), 2, axis=-1).astype(np.float32)
    sin = np.repeat(np.sin(pos), 2, axis=-1).astype(np.float32)
    sign = np.where(np.arange(DH) % 2 == 0, -1.0, 1.0).astype(np.float32)
    sin = sin * sign[None, :]
    return np.stack([cos, sin]).astype(np.float32)


_TABLES = _rope_tables()


def pallas_dist_rope_attn_htp_bs_b2_sq512_d1024_hq8_dh128_kernel(x, Wq, Wk, Wv, Wo):
    f32, bf16 = jnp.float32, jnp.bfloat16
    MESH = pl.DeviceIdType.MESH

    def body(x_hbm, wq_hbm, wk_hbm, wv_hbm, wo_hbm, tab_hbm, out_ref,
             tab_ref,             xst, wst, wb, x_all, ctx, ctx0, sbuf, rbuf,
             x_sems, w_sems, ag_s, ag_r, rs_s, rs_r):
        me = lax.axis_index("i")
        right = lax.rem(me + 1, N_DEV)
        left = lax.rem(me + 3, N_DEV)
        diag = lax.rem(me + 2, N_DEV)

        NP = HL // 2
        PW = 2 * DH
        w_hbm = (wq_hbm, wk_hbm, wv_hbm)

        def x_ld(b):
            return pltpu.make_async_copy(x_hbm.at[b], xst.at[b], x_sems.at[b])

        def w_ld(i, hp):
            cols = pl.ds(hp * PW, PW)
            return pltpu.make_async_copy(w_hbm[i].at[:, cols], wst.at[i, :, cols],
                                         w_sems.at[i * NP + hp])

        wo_ld = pltpu.make_async_copy(wo_hbm, wst.at[3], w_sems.at[3 * NP])

        def ag(src_slot, dst_slot, dev):
            return pltpu.make_async_remote_copy(
                src_ref=x_all.at[src_slot], dst_ref=x_all.at[dst_slot],
                send_sem=ag_s.at[dst_slot - 1], recv_sem=ag_r.at[dst_slot - 1],
                device_id=(dev,), device_id_type=MESH)

        def rs(step, dev):
            return pltpu.make_async_remote_copy(
                src_ref=sbuf.at[step - 1], dst_ref=rbuf.at[step - 1],
                send_sem=rs_s.at[step - 1], recv_sem=rs_r.at[step - 1],
                device_id=(dev,), device_id_type=MESH)

        even = (lax.broadcasted_iota(jnp.int32, (S, DH), 1) % 2) == 0

        def rope(t, c, s):
            sw = jnp.where(even, pltpu.roll(t, DH - 1, 1), pltpu.roll(t, 1, 1))
            return (t * c + sw * s).astype(bf16)

        def attention(slot, ctx, first=False):
            xb = x_all[slot]
            for hp in range(NP):
                cols = slice(hp * PW, (hp + 1) * PW)
                qkv = []
                for i in range(3):
                    if first:
                        ld_wait(2 if (i == 2 and hp < 2) else 1)
                        w = wst[i, :, cols]
                        if i == 0:
                            w = w * (SCALE * LOG2E)
                        wb[i, :, cols] = w.astype(bf16)
                    qkv.append(jnp.dot(xb, wb[i, :, cols], preferred_element_type=f32))
                if first and hp == 1:
                    x_all[7] = xst[1].astype(bf16)
                    ag(7, 2, left).start()
                    ag(7, 6, right).start()
                q2, k2, v2 = qkv[0], qkv[1], qkv[2].astype(bf16)
                for j in range(2):
                    h = hp * 2 + j
                    hs = slice(j * DH, (j + 1) * DH)
                    q = rope(q2[:, hs], tab_ref[0], tab_ref[1])
                    k = rope(k2[:, hs], tab_ref[0], tab_ref[1])
                    sc = lax.dot_general(q, k, (((1,), (1,)), ((), ())),
                                         preferred_element_type=f32)
                    m = jnp.max(sc, axis=-1, keepdims=True)
                    p = jnp.exp2(sc - m)
                    l = jnp.sum(p, axis=-1, keepdims=True)
                    o = jnp.dot(p.astype(bf16), v2[:, hs], preferred_element_type=f32)
                    ctx[:, h * DH:(h + 1) * DH] = (o / l).astype(bf16)

        tab_ld = pltpu.make_async_copy(tab_hbm, tab_ref, x_sems.at[2])
        loads = [x_ld(0), w_ld(0, 0), w_ld(1, 0), w_ld(2, 0), tab_ld,
                 w_ld(0, 1), w_ld(1, 1), w_ld(2, 1), x_ld(1)]
        loads += [w_ld(i, hp) for hp in (2, 3) for i in range(3)] + [wo_ld]
        pos = [0, 2]

        def ld_wait(n=1):
            for _ in range(n):
                loads[pos[0]].wait()
                pos[0] += 1
            while pos[1] < min(pos[0] + 4, len(loads)):
                loads[pos[1]].start()
                pos[1] += 1

        for c in loads[:2]:
            c.start()
        bar = pltpu.get_barrier_semaphore()
        for d in (left, right):
            pl.semaphore_signal(bar, inc=1, device_id=(d,), device_id_type=MESH)
        ld_wait()
        x_all[0] = xst[0].astype(bf16)
        pl.semaphore_wait(bar, 2)
        ag(0, 1, right).start()
        ag(0, 4, left).start()
        attention(0, ctx0, first=True)
        ld_wait()
        wb[3] = wst[3].astype(bf16)

        def step_fn(s, carry):
            ag(0, s, me).wait_recv()

            @pl.when(s == 1)
            def _():
                ag(1, 3, right).start()

            @pl.when(s == 2)
            def _():
                ag(2, 5, left).start()

            attention(s, ctx)
            relay = jnp.logical_or(s == 4, s == 6)

            part = jnp.dot(ctx[...], wb[3], preferred_element_type=f32)
            sbuf[s - 1] = part.astype(bf16)

            @pl.when(relay)
            def _():
                rs(s - 1, me).wait_recv()
                sbuf[s - 1] = (part + rbuf[s - 2].astype(f32)).astype(bf16)

            to_right = jnp.logical_and(s >= 2, s <= 4)
            rs(s, jnp.where(to_right, right, left)).start()
            return carry

        lax.fori_loop(1, 7, step_fn, 0)

        for t in (1, 4):
            rs(t, me).wait_recv()
        part = jnp.dot(ctx0[...], wb[3], preferred_element_type=f32)
        out_ref[0] = part + (rbuf[0].astype(f32) + rbuf[3].astype(f32))
        attention(7, ctx)
        for t in (2, 6):
            rs(t, me).wait_recv()
        part = jnp.dot(ctx[...], wb[3], preferred_element_type=f32)
        out_ref[1] = part + (rbuf[1].astype(f32) + rbuf[5].astype(f32))

        for t in range(1, 7):
            ag(0, t, me).wait_send()
            rs(t, me).wait_send()

    any_spec = pl.BlockSpec(memory_space=pl.ANY)
    return pl.pallas_call(
        body,
        out_shape=jax.ShapeDtypeStruct((BL, S, D), f32),
        in_specs=[any_spec] * 6,
        out_specs=pl.BlockSpec((BL, S, D), lambda: (0, 0, 0)),
        scratch_shapes=[
            pltpu.VMEM((2, S, DH), f32),
            pltpu.VMEM((BL, S, D), f32),
            pltpu.VMEM((4, D, D), f32),
            pltpu.VMEM((4, D, D), bf16),
            pltpu.VMEM((8, S, D), bf16),
            pltpu.VMEM((S, D), bf16),
            pltpu.VMEM((S, D), bf16),
            pltpu.VMEM((6, S, D), bf16),
            pltpu.VMEM((6, S, D), bf16),
            pltpu.SemaphoreType.DMA((3,)),
            pltpu.SemaphoreType.DMA((13,)),
            pltpu.SemaphoreType.DMA((6,)),
            pltpu.SemaphoreType.DMA((6,)),
            pltpu.SemaphoreType.DMA((6,)),
            pltpu.SemaphoreType.DMA((6,)),
        ],
        compiler_params=pltpu.CompilerParams(collective_id=0, vmem_limit_bytes=100 * 1024 * 1024),
    )(x, Wq, Wk, Wv, Wo, jnp.asarray(_TABLES))
```

```python
import jax
import jax.numpy as jnp
import numpy as np
from jax import lax
from jax.experimental import pallas as pl
from jax.experimental.pallas import tpu as pltpu

N_DEV = 4
BL, S, D = 2, 512, 1024
HL, DH = 8, 128
SCALE = 0.08838834764831843
LOG2E = 1.4426950408889634


def _rope_tables():
    inv = 1.0 / (10000.0 ** (np.arange(0, DH, 2) / DH))
    pos = np.arange(S)[:, None] * inv[None, :]
    cos = np.repeat(np.cos(pos), 2, axis=-1).astype(np.float32)
    sin = np.repeat(np.sin(pos), 2, axis=-1).astype(np.float32)
    sign = np.where(np.arange(DH) % 2 == 0, -1.0, 1.0).astype(np.float32)
    sin = sin * sign[None, :]
    return np.stack([cos, sin]).astype(np.float32)


_TABLES = _rope_tables()


def pallas_dist_rope_attn_htp_bs_b2_sq512_d1024_hq8_dh128_kernel(x, Wq, Wk, Wv, Wo):
    f32, bf16 = jnp.float32, jnp.bfloat16
    MESH = pl.DeviceIdType.MESH

    def body(x_hbm, wq_hbm, wk_hbm, wv_hbm, wo_hbm, tab_hbm, out_ref,
             tab_ref,             xst, wst, ws, wo, xs, x_all, ctx, ctx0, sbuf, rbuf,
             x_sems, w_sems, ag_s, ag_r, rs_s, rs_r):
        me = lax.axis_index("i")
        right = lax.rem(me + 1, N_DEV)
        left = lax.rem(me + 3, N_DEV)
        diag = lax.rem(me + 2, N_DEV)

        NP = HL // 2
        PW = 2 * DH
        HS, HD = S // 2, D // 2
        w_hbm = (wq_hbm, wk_hbm, wv_hbm)

        def x_ld(b):
            return pltpu.make_async_copy(x_hbm.at[b], xst.at[b], x_sems.at[b])

        def w_ld(i, hp):
            cols = pl.ds(hp * PW, PW)
            return pltpu.make_async_copy(w_hbm[i].at[:, cols], wst.at[i, :, cols],
                                         w_sems.at[i * NP + hp])

        wo_ld = pltpu.make_async_copy(wo_hbm, wst.at[3], w_sems.at[3 * NP])

        def ag(src_slot, dst_slot, dev):
            return pltpu.make_async_remote_copy(
                src_ref=x_all.at[src_slot], dst_ref=x_all.at[dst_slot],
                send_sem=ag_s.at[dst_slot - 1], recv_sem=ag_r.at[dst_slot - 1],
                device_id=(dev,), device_id_type=MESH)

        def rs(step, dev):
            return pltpu.make_async_remote_copy(
                src_ref=sbuf.at[step - 1], dst_ref=rbuf.at[step - 1],
                send_sem=rs_s.at[step - 1], recv_sem=rs_r.at[step - 1],
                device_id=(dev,), device_id_type=MESH)

        even = (lax.broadcasted_iota(jnp.int32, (S, DH), 1) % 2) == 0

        def rope(t, c, s):
            sw = jnp.where(even, pltpu.roll(t, DH - 1, 1), pltpu.roll(t, 1, 1))
            return (t * c + sw * s).astype(bf16)

        def attention(slot, ctx, first=False):
            a11 = x_all[slot, :HS, :HD].astype(f32)
            a12 = x_all[slot, :HS, HD:].astype(f32)
            a21 = x_all[slot, HS:, :HD].astype(f32)
            a22 = x_all[slot, HS:, HD:].astype(f32)
            for n, t in enumerate((a11 + a22, a21 + a22, a11 + a12, a21 - a11, a12 - a22)):
                xs[n] = t.astype(bf16)
            for hp in range(NP):
                if first:
                    for i in range(3):
                        ld_wait(2 if (i == 2 and hp < 2) else 1)
                        c0 = slice(hp * PW, hp * PW + DH)
                        c1 = slice(hp * PW + DH, (hp + 1) * PW)
                        b11, b12 = wst[i, :HD, c0], wst[i, :HD, c1]
                        b21, b22 = wst[i, HD:, c0], wst[i, HD:, c1]
                        if i == 0:
                            b11, b12, b21, b22 = (t * (SCALE * LOG2E) for t in (b11, b12, b21, b22))
                        for n, t in enumerate((b11 + b22, b11, b12 - b22, b21 - b11,
                                               b22, b11 + b12, b21 + b22)):
                            ws[hp, n, :, i * DH:(i + 1) * DH] = t.astype(bf16)
                if first and hp == 1:
                    x_all[7] = xst[1].astype(bf16)
                    ag(7, 2, left).start()
                    ag(7, 6, right).start()
                lhs = (xs[0], xs[1], x_all[slot, :HS, :HD], x_all[slot, HS:, HD:], xs[2], xs[3], xs[4])
                m1, m2, m3, m4, m5, m6, m7 = (
                    jnp.dot(lhs[n], ws[hp, n], preferred_element_type=f32) for n in range(7))
                heads = (jnp.concatenate([(m1 + m4) + (m7 - m5), m2 + m4], axis=0),
                         jnp.concatenate([m3 + m5, (m1 - m2) + (m3 + m6)], axis=0))
                for j in range(2):
                    h = hp * 2 + j
                    q = rope(heads[j][:, :DH], tab_ref[0], tab_ref[1])
                    k = rope(heads[j][:, DH:2 * DH], tab_ref[0], tab_ref[1])
                    v = heads[j][:, 2 * DH:].astype(bf16)
                    sc = lax.dot_general(q, k, (((1,), (1,)), ((), ())),
                                         preferred_element_type=f32)
                    m = jnp.max(sc, axis=-1, keepdims=True)
                    p = jnp.exp2(sc - m)
                    l = jnp.sum(p, axis=-1, keepdims=True)
                    o = jnp.dot(p.astype(bf16), v, preferred_element_type=f32)
                    ctx[:, h * DH:(h + 1) * DH] = (o / l).astype(bf16)

        tab_ld = pltpu.make_async_copy(tab_hbm, tab_ref, x_sems.at[2])
        loads = [x_ld(0), w_ld(0, 0), w_ld(1, 0), w_ld(2, 0), tab_ld,
                 w_ld(0, 1), w_ld(1, 1), w_ld(2, 1), x_ld(1)]
        loads += [w_ld(i, hp) for hp in (2, 3) for i in range(3)] + [wo_ld]
        pos = [0, 2]

        def ld_wait(n=1):
            for _ in range(n):
                loads[pos[0]].wait()
                pos[0] += 1
            while pos[1] < min(pos[0] + 4, len(loads)):
                loads[pos[1]].start()
                pos[1] += 1

        for c in loads[:2]:
            c.start()
        bar = pltpu.get_barrier_semaphore()
        for d in (left, right):
            pl.semaphore_signal(bar, inc=1, device_id=(d,), device_id_type=MESH)
        ld_wait()
        x_all[0] = xst[0].astype(bf16)
        pl.semaphore_wait(bar, 2)
        ag(0, 1, right).start()
        ag(0, 4, left).start()
        attention(0, ctx0, first=True)
        ld_wait()
        wo[...] = wst[3].astype(bf16)

        def step_fn(s, carry):
            ag(0, s, me).wait_recv()

            @pl.when(s == 1)
            def _():
                ag(1, 3, right).start()

            @pl.when(s == 2)
            def _():
                ag(2, 5, left).start()

            attention(s, ctx)
            relay = jnp.logical_or(s == 4, s == 6)

            part = jnp.dot(ctx[...], wo[...], preferred_element_type=f32)
            sbuf[s - 1] = part.astype(bf16)

            @pl.when(relay)
            def _():
                rs(s - 1, me).wait_recv()
                sbuf[s - 1] = (part + rbuf[s - 2].astype(f32)).astype(bf16)

            to_right = jnp.logical_and(s >= 2, s <= 4)
            rs(s, jnp.where(to_right, right, left)).start()
            return carry

        lax.fori_loop(1, 7, step_fn, 0)

        for t in (1, 4):
            rs(t, me).wait_recv()
        part = jnp.dot(ctx0[...], wo[...], preferred_element_type=f32)
        out_ref[0] = part + (rbuf[0].astype(f32) + rbuf[3].astype(f32))
        attention(7, ctx)
        for t in (2, 6):
            rs(t, me).wait_recv()
        part = jnp.dot(ctx[...], wo[...], preferred_element_type=f32)
        out_ref[1] = part + (rbuf[1].astype(f32) + rbuf[5].astype(f32))

        for t in range(1, 7):
            ag(0, t, me).wait_send()
            rs(t, me).wait_send()

    any_spec = pl.BlockSpec(memory_space=pl.ANY)
    return pl.pallas_call(
        body,
        out_shape=jax.ShapeDtypeStruct((BL, S, D), f32),
        in_specs=[any_spec] * 6,
        out_specs=pl.BlockSpec((BL, S, D), lambda: (0, 0, 0)),
        scratch_shapes=[
            pltpu.VMEM((2, S, DH), f32),
            pltpu.VMEM((BL, S, D), f32),
            pltpu.VMEM((4, D, D), f32),
            pltpu.VMEM((HL // 2, 7, D // 2, 3 * DH), bf16),
            pltpu.VMEM((D, D), bf16),
            pltpu.VMEM((5, S // 2, D // 2), bf16),
            pltpu.VMEM((8, S, D), bf16),
            pltpu.VMEM((S, D), bf16),
            pltpu.VMEM((S, D), bf16),
            pltpu.VMEM((6, S, D), bf16),
            pltpu.VMEM((6, S, D), bf16),
            pltpu.SemaphoreType.DMA((3,)),
            pltpu.SemaphoreType.DMA((13,)),
            pltpu.SemaphoreType.DMA((6,)),
            pltpu.SemaphoreType.DMA((6,)),
            pltpu.SemaphoreType.DMA((6,)),
            pltpu.SemaphoreType.DMA((6,)),
        ],
        compiler_params=pltpu.CompilerParams(collective_id=0, vmem_limit_bytes=100 * 1024 * 1024),
    )(x, Wq, Wk, Wv, Wo, jnp.asarray(_TABLES))
```

```python
import jax
import jax.numpy as jnp
import numpy as np
from jax import lax
from jax.experimental import pallas as pl
from jax.experimental.pallas import tpu as pltpu

N_DEV = 4
BL, S, D = 2, 512, 1024
HL, DH = 8, 128
SCALE = 0.08838834764831843
LOG2E = 1.4426950408889634


def _rope_tables():
    inv = 1.0 / (10000.0 ** (np.arange(0, DH, 2) / DH))
    pos = np.arange(S)[:, None] * inv[None, :]
    cos = np.repeat(np.cos(pos), 2, axis=-1).astype(np.float32)
    sin = np.repeat(np.sin(pos), 2, axis=-1).astype(np.float32)
    sign = np.where(np.arange(DH) % 2 == 0, -1.0, 1.0).astype(np.float32)
    sin = sin * sign[None, :]
    return np.stack([cos, sin]).astype(np.float32)


_TABLES = _rope_tables()


def pallas_dist_rope_attn_htp_bs_b2_sq512_d1024_hq8_dh128_kernel(x, Wq, Wk, Wv, Wo):
    f32, bf16 = jnp.float32, jnp.bfloat16
    MESH = pl.DeviceIdType.MESH

    def body(x_hbm, wq_hbm, wk_hbm, wv_hbm, wo_hbm, tab_hbm, out_ref,
             tab_ref,             xst, wst, ws, wo, xs, x_all, ctx, ctx0, sbuf, rbuf,
             x_sems, w_sems, ag_s, ag_r, rs_s, rs_r):
        me = lax.axis_index("i")
        right = lax.rem(me + 1, N_DEV)
        left = lax.rem(me + 3, N_DEV)
        diag = lax.rem(me + 2, N_DEV)

        NP = HL // 2
        PW = 2 * DH
        w_hbm = (wq_hbm, wk_hbm, wv_hbm)

        def x_ld(b):
            return pltpu.make_async_copy(x_hbm.at[b], xst.at[b], x_sems.at[b])

        def w_ld(i, hp):
            cols = pl.ds(hp * PW, PW)
            return pltpu.make_async_copy(w_hbm[i].at[:, cols], wst.at[i, :, cols],
                                         w_sems.at[i * NP + hp])

        wo_ld = pltpu.make_async_copy(wo_hbm, wst.at[3], w_sems.at[3 * NP])

        def ag(src_slot, dst_slot, dev):
            return pltpu.make_async_remote_copy(
                src_ref=x_all.at[src_slot], dst_ref=x_all.at[dst_slot],
                send_sem=ag_s.at[dst_slot - 1], recv_sem=ag_r.at[dst_slot - 1],
                device_id=(dev,), device_id_type=MESH)

        def rs(step, dev):
            return pltpu.make_async_remote_copy(
                src_ref=sbuf.at[step - 1], dst_ref=rbuf.at[step - 1],
                send_sem=rs_s.at[step - 1], recv_sem=rs_r.at[step - 1],
                device_id=(dev,), device_id_type=MESH)

        even = (lax.broadcasted_iota(jnp.int32, (S, DH), 1) % 2) == 0

        def rope(t, c, s):
            sw = jnp.where(even, pltpu.roll(t, DH - 1, 1), pltpu.roll(t, 1, 1))
            return (t * c + sw * s).astype(bf16)

        HS, HD = S // 2, D // 2

        def rhs_terms(b11, b12, b21, b22):
            return b11 + b22, b11, b12 - b22, b21 - b11, b22, b11 + b12, b21 + b22

        def out_proj(c):
            a11, a12, a21, a22 = c[:HS, :HD], c[:HS, HD:], c[HS:, :HD], c[HS:, HD:]
            f11, f12, f21, f22 = (t.astype(f32) for t in (a11, a12, a21, a22))
            lhs = ((f11 + f22).astype(bf16), (f21 + f22).astype(bf16), a11, a22,
                   (f11 + f12).astype(bf16), (f21 - f11).astype(bf16), (f12 - f22).astype(bf16))
            m1, m2, m3, m4, m5, m6, m7 = (
                jnp.dot(lhs[n], wo[n], preferred_element_type=f32) for n in range(7))
            return jnp.concatenate(
                [jnp.concatenate([(m1 + m4) + (m7 - m5), m3 + m5], axis=1),
                 jnp.concatenate([m2 + m4, (m1 - m2) + (m3 + m6)], axis=1)], axis=0)

        def attention(slot, ctx, first=False):
            a11 = x_all[slot, :HS, :HD].astype(f32)
            a12 = x_all[slot, :HS, HD:].astype(f32)
            a21 = x_all[slot, HS:, :HD].astype(f32)
            a22 = x_all[slot, HS:, HD:].astype(f32)
            for n, t in enumerate((a11 + a22, a21 + a22, a11 + a12, a21 - a11, a12 - a22)):
                xs[n] = t.astype(bf16)
            for hp in range(NP):
                if first:
                    for i in range(3):
                        ld_wait(2 if (i == 2 and hp < 2) else 1)
                        c0 = slice(hp * PW, hp * PW + DH)
                        c1 = slice(hp * PW + DH, (hp + 1) * PW)
                        b11, b12 = wst[i, :HD, c0], wst[i, :HD, c1]
                        b21, b22 = wst[i, HD:, c0], wst[i, HD:, c1]
                        if i == 0:
                            b11, b12, b21, b22 = (t * (SCALE * LOG2E) for t in (b11, b12, b21, b22))
                        for n, t in enumerate(rhs_terms(b11, b12, b21, b22)):
                            ws[hp, n, :, i * DH:(i + 1) * DH] = t.astype(bf16)
                if first and hp == 1:
                    x_all[7] = xst[1].astype(bf16)
                    ag(7, 2, left).start()
                    ag(7, 6, right).start()
                lhs = (xs[0], xs[1], x_all[slot, :HS, :HD], x_all[slot, HS:, HD:], xs[2], xs[3], xs[4])
                m1, m2, m3, m4, m5, m6, m7 = (
                    jnp.dot(lhs[n], ws[hp, n], preferred_element_type=f32) for n in range(7))
                heads = (jnp.concatenate([(m1 + m4) + (m7 - m5), m2 + m4], axis=0),
                         jnp.concatenate([m3 + m5, (m1 - m2) + (m3 + m6)], axis=0))
                for j in range(2):
                    h = hp * 2 + j
                    q = rope(heads[j][:, :DH], tab_ref[0], tab_ref[1])
                    k = rope(heads[j][:, DH:2 * DH], tab_ref[0], tab_ref[1])
                    v = heads[j][:, 2 * DH:].astype(bf16)
                    sc = lax.dot_general(q, k, (((1,), (1,)), ((), ())),
                                         preferred_element_type=f32)
                    m = jnp.max(sc, axis=-1, keepdims=True)
                    p = jnp.exp2(sc - m)
                    l = jnp.sum(p, axis=-1, keepdims=True)
                    o = jnp.dot(p.astype(bf16), v, preferred_element_type=f32)
                    ctx[:, h * DH:(h + 1) * DH] = (o / l).astype(bf16)

        tab_ld = pltpu.make_async_copy(tab_hbm, tab_ref, x_sems.at[2])
        loads = [x_ld(0), w_ld(0, 0), w_ld(1, 0), w_ld(2, 0), tab_ld,
                 w_ld(0, 1), w_ld(1, 1), w_ld(2, 1), x_ld(1)]
        loads += [w_ld(i, hp) for hp in (2, 3) for i in range(3)] + [wo_ld]
        pos = [0, 2]

        def ld_wait(n=1):
            for _ in range(n):
                loads[pos[0]].wait()
                pos[0] += 1
            while pos[1] < min(pos[0] + 4, len(loads)):
                loads[pos[1]].start()
                pos[1] += 1

        for c in loads[:2]:
            c.start()
        bar = pltpu.get_barrier_semaphore()
        for d in (left, right):
            pl.semaphore_signal(bar, inc=1, device_id=(d,), device_id_type=MESH)
        ld_wait()
        x_all[0] = xst[0].astype(bf16)
        pl.semaphore_wait(bar, 2)
        ag(0, 1, right).start()
        ag(0, 4, left).start()
        attention(0, ctx0, first=True)
        ld_wait()
        for n, t in enumerate(rhs_terms(wst[3, :HD, :HD], wst[3, :HD, HD:],
                                        wst[3, HD:, :HD], wst[3, HD:, HD:])):
            wo[n] = t.astype(bf16)

        def step_fn(s, carry):
            ag(0, s, me).wait_recv()

            @pl.when(s == 1)
            def _():
                ag(1, 3, right).start()

            @pl.when(s == 2)
            def _():
                ag(2, 5, left).start()

            attention(s, ctx)
            relay = jnp.logical_or(s == 4, s == 6)

            part = out_proj(ctx)
            sbuf[s - 1] = part.astype(bf16)

            @pl.when(relay)
            def _():
                rs(s - 1, me).wait_recv()
                sbuf[s - 1] = (part + rbuf[s - 2].astype(f32)).astype(bf16)

            to_right = jnp.logical_and(s >= 2, s <= 4)
            rs(s, jnp.where(to_right, right, left)).start()
            return carry

        lax.fori_loop(1, 7, step_fn, 0)

        for t in (1, 4):
            rs(t, me).wait_recv()
        part = out_proj(ctx0)
        out_ref[0] = part + (rbuf[0].astype(f32) + rbuf[3].astype(f32))
        attention(7, ctx)
        for t in (2, 6):
            rs(t, me).wait_recv()
        part = out_proj(ctx)
        out_ref[1] = part + (rbuf[1].astype(f32) + rbuf[5].astype(f32))

        for t in range(1, 7):
            ag(0, t, me).wait_send()
            rs(t, me).wait_send()

    any_spec = pl.BlockSpec(memory_space=pl.ANY)
    return pl.pallas_call(
        body,
        out_shape=jax.ShapeDtypeStruct((BL, S, D), f32),
        in_specs=[any_spec] * 6,
        out_specs=pl.BlockSpec((BL, S, D), lambda: (0, 0, 0)),
        scratch_shapes=[
            pltpu.VMEM((2, S, DH), f32),
            pltpu.VMEM((BL, S, D), f32),
            pltpu.VMEM((4, D, D), f32),
            pltpu.VMEM((HL // 2, 7, D // 2, 3 * DH), bf16),
            pltpu.VMEM((7, D // 2, D // 2), bf16),
            pltpu.VMEM((5, S // 2, D // 2), bf16),
            pltpu.VMEM((8, S, D), bf16),
            pltpu.VMEM((S, D), bf16),
            pltpu.VMEM((S, D), bf16),
            pltpu.VMEM((6, S, D), bf16),
            pltpu.VMEM((6, S, D), bf16),
            pltpu.SemaphoreType.DMA((3,)),
            pltpu.SemaphoreType.DMA((13,)),
            pltpu.SemaphoreType.DMA((6,)),
            pltpu.SemaphoreType.DMA((6,)),
            pltpu.SemaphoreType.DMA((6,)),
            pltpu.SemaphoreType.DMA((6,)),
        ],
        compiler_params=pltpu.CompilerParams(collective_id=0, vmem_limit_bytes=100 * 1024 * 1024),
    )(x, Wq, Wk, Wv, Wo, jnp.asarray(_TABLES))
```

```python
import jax
import jax.numpy as jnp
import numpy as np
from jax import lax
from jax.experimental import pallas as pl
from jax.experimental.pallas import tpu as pltpu

N_DEV = 4
BL, S, D = 2, 512, 1024
HL, DH = 8, 128
SCALE = 0.08838834764831843
LOG2E = 1.4426950408889634


def _rope_tables():
    inv = 1.0 / (10000.0 ** (np.arange(0, DH, 2) / DH))
    pos = np.arange(S)[:, None] * inv[None, :]
    cos = np.repeat(np.cos(pos), 2, axis=-1).astype(np.float32)
    sin = np.repeat(np.sin(pos), 2, axis=-1).astype(np.float32)
    sign = np.where(np.arange(DH) % 2 == 0, -1.0, 1.0).astype(np.float32)
    sin = sin * sign[None, :]
    return np.stack([cos, sin]).astype(np.float32)


_TABLES = _rope_tables()


def pallas_dist_rope_attn_htp_bs_b2_sq512_d1024_hq8_dh128_kernel(x, Wq, Wk, Wv, Wo):
    f32, bf16 = jnp.float32, jnp.bfloat16
    MESH = pl.DeviceIdType.MESH

    def body(x_hbm, wq_hbm, wk_hbm, wv_hbm, wo_hbm, tab_hbm, out_ref,
             tab_ref,             xst, wst, ws, wo, xs, x_all, ctx, ctx0, sbuf, rbuf,
             x_sems, w_sems, ag_s, ag_r, rs_s, rs_r):
        me = lax.axis_index("i")
        right = lax.rem(me + 1, N_DEV)
        left = lax.rem(me + 3, N_DEV)
        diag = lax.rem(me + 2, N_DEV)

        NP = HL // 2
        PW = 2 * DH
        w_hbm = (wq_hbm, wk_hbm, wv_hbm)

        def x_ld(b):
            return pltpu.make_async_copy(x_hbm.at[b], xst.at[b], x_sems.at[b])

        def w_ld(i, hp):
            cols = pl.ds(hp * PW, PW)
            return pltpu.make_async_copy(w_hbm[i].at[:, cols], wst.at[i, :, cols],
                                         w_sems.at[i * NP + hp])

        wo_ld = pltpu.make_async_copy(wo_hbm, wst.at[3], w_sems.at[3 * NP])

        def ag(src_slot, dst_slot, dev):
            return pltpu.make_async_remote_copy(
                src_ref=x_all.at[src_slot], dst_ref=x_all.at[dst_slot],
                send_sem=ag_s.at[dst_slot - 1], recv_sem=ag_r.at[dst_slot - 1],
                device_id=(dev,), device_id_type=MESH)

        def rs(step, dev):
            return pltpu.make_async_remote_copy(
                src_ref=sbuf.at[step - 1], dst_ref=rbuf.at[step - 1],
                send_sem=rs_s.at[step - 1], recv_sem=rs_r.at[step - 1],
                device_id=(dev,), device_id_type=MESH)

        even = (lax.broadcasted_iota(jnp.int32, (S, DH), 1) % 2) == 0

        def rope(t, c, s):
            sw = jnp.where(even, pltpu.roll(t, DH - 1, 1), pltpu.roll(t, 1, 1))
            return (t * c + sw * s).astype(bf16)

        HS, HD = S // 2, D // 2

        def rhs_terms(b11, b12, b21, b22):
            return b11 + b22, b11, b12 - b22, b21 - b11, b22, b11 + b12, b21 + b22

        def out_proj(c):
            a11, a12, a21, a22 = c[:HS, :HD], c[:HS, HD:], c[HS:, :HD], c[HS:, HD:]
            f11, f12, f21, f22 = (t.astype(f32) for t in (a11, a12, a21, a22))
            lhs = ((f11 + f22).astype(bf16), (f21 + f22).astype(bf16), a11, a22,
                   (f11 + f12).astype(bf16), (f21 - f11).astype(bf16), (f12 - f22).astype(bf16))
            m1, m2, m3, m4, m5, m6, m7 = (
                jnp.dot(lhs[n], wo[n], preferred_element_type=f32) for n in range(7))
            return jnp.concatenate(
                [jnp.concatenate([(m1 + m4) + (m7 - m5), m3 + m5], axis=1),
                 jnp.concatenate([m2 + m4, (m1 - m2) + (m3 + m6)], axis=1)], axis=0)

        def prep_w(hp):
            for i in range(3):
                ld_wait(2 if (i == 2 and hp == 0) else 1)
                c0 = slice(hp * PW, hp * PW + DH)
                c1 = slice(hp * PW + DH, (hp + 1) * PW)
                b11, b12 = wst[i, :HD, c0], wst[i, :HD, c1]
                b21, b22 = wst[i, HD:, c0], wst[i, HD:, c1]
                if i == 0:
                    b11, b12, b21, b22 = (t * (SCALE * LOG2E) for t in (b11, b12, b21, b22))
                for n, t in enumerate(rhs_terms(b11, b12, b21, b22)):
                    ws[hp, n, :, i * DH:(i + 1) * DH] = t.astype(bf16)

        def attention(slot, ctx, first=False):
            a11 = x_all[slot, :HS, :HD].astype(f32)
            a12 = x_all[slot, :HS, HD:].astype(f32)
            a21 = x_all[slot, HS:, :HD].astype(f32)
            a22 = x_all[slot, HS:, HD:].astype(f32)
            for n, t in enumerate((a11 + a22, a21 + a22, a11 + a12, a21 - a11, a12 - a22)):
                xs[n] = t.astype(bf16)
            if first:
                prep_w(0)
            for hp in range(NP):
                lhs = (xs[0], xs[1], x_all[slot, :HS, :HD], x_all[slot, HS:, HD:], xs[2], xs[3], xs[4])
                m1, m2, m3, m4, m5, m6, m7 = (
                    jnp.dot(lhs[n], ws[hp, n], preferred_element_type=f32) for n in range(7))
                heads = (jnp.concatenate([(m1 + m4) + (m7 - m5), m2 + m4], axis=0),
                         jnp.concatenate([m3 + m5, (m1 - m2) + (m3 + m6)], axis=0))
                qkv = [(rope(t[:, :DH], tab_ref[0], tab_ref[1]),
                        rope(t[:, DH:2 * DH], tab_ref[0], tab_ref[1]),
                        t[:, 2 * DH:].astype(bf16)) for t in heads]
                if first and hp + 1 < NP:
                    prep_w(hp + 1)
                for j in range(2):
                    h = hp * 2 + j
                    q, k, v = qkv[j]
                    sc = lax.dot_general(q, k, (((1,), (1,)), ((), ())),
                                         preferred_element_type=f32)
                    m = jnp.max(sc, axis=-1, keepdims=True)
                    p = jnp.exp2(sc - m)
                    l = jnp.sum(p, axis=-1, keepdims=True)
                    o = jnp.dot(p.astype(bf16), v, preferred_element_type=f32)
                    ctx[:, h * DH:(h + 1) * DH] = (o / l).astype(bf16)

        loads = [x_ld(0), w_ld(0, 0), w_ld(1, 0), w_ld(2, 0),
                 pltpu.make_async_copy(tab_hbm, tab_ref, x_sems.at[2])]
        loads += [w_ld(i, hp) for hp in (1, 2, 3) for i in range(3)] + [x_ld(1), wo_ld]
        pos = [0, 2]

        def ld_wait(n=1):
            for _ in range(n):
                loads[pos[0]].wait()
                pos[0] += 1
            while pos[1] < min(pos[0] + 4, len(loads)):
                loads[pos[1]].start()
                pos[1] += 1

        for c in loads[:2]:
            c.start()
        bar = pltpu.get_barrier_semaphore()
        for d in (left, right):
            pl.semaphore_signal(bar, inc=1, device_id=(d,), device_id_type=MESH)
        ld_wait()
        x_all[0] = xst[0].astype(bf16)
        pl.semaphore_wait(bar, 2)
        ag(0, 1, right).start()
        ag(0, 4, left).start()
        attention(0, ctx0, first=True)
        ld_wait(2)
        x_all[7] = xst[1].astype(bf16)
        ag(7, 2, left).start()
        ag(7, 6, right).start()
        for n, t in enumerate(rhs_terms(wst[3, :HD, :HD], wst[3, :HD, HD:],
                                        wst[3, HD:, :HD], wst[3, HD:, HD:])):
            wo[n] = t.astype(bf16)

        def step_fn(s, carry):
            ag(0, s, me).wait_recv()

            @pl.when(s == 1)
            def _():
                ag(1, 3, right).start()

            @pl.when(s == 2)
            def _():
                ag(2, 5, left).start()

            attention(s, ctx)
            relay = jnp.logical_or(s == 4, s == 6)

            part = out_proj(ctx)
            sbuf[s - 1] = part.astype(bf16)

            @pl.when(relay)
            def _():
                rs(s - 1, me).wait_recv()
                sbuf[s - 1] = (part + rbuf[s - 2].astype(f32)).astype(bf16)

            to_right = jnp.logical_and(s >= 2, s <= 4)
            rs(s, jnp.where(to_right, right, left)).start()
            return carry

        lax.fori_loop(1, 7, step_fn, 0)

        for t in (1, 4):
            rs(t, me).wait_recv()
        part = out_proj(ctx0)
        out_ref[0] = part + (rbuf[0].astype(f32) + rbuf[3].astype(f32))
        attention(7, ctx)
        for t in (2, 6):
            rs(t, me).wait_recv()
        part = out_proj(ctx)
        out_ref[1] = part + (rbuf[1].astype(f32) + rbuf[5].astype(f32))

        for t in range(1, 7):
            ag(0, t, me).wait_send()
            rs(t, me).wait_send()

    any_spec = pl.BlockSpec(memory_space=pl.ANY)
    return pl.pallas_call(
        body,
        out_shape=jax.ShapeDtypeStruct((BL, S, D), f32),
        in_specs=[any_spec] * 6,
        out_specs=pl.BlockSpec((BL, S, D), lambda: (0, 0, 0)),
        scratch_shapes=[
            pltpu.VMEM((2, S, DH), f32),
            pltpu.VMEM((BL, S, D), f32),
            pltpu.VMEM((4, D, D), f32),
            pltpu.VMEM((HL // 2, 7, D // 2, 3 * DH), bf16),
            pltpu.VMEM((7, D // 2, D // 2), bf16),
            pltpu.VMEM((5, S // 2, D // 2), bf16),
            pltpu.VMEM((8, S, D), bf16),
            pltpu.VMEM((S, D), bf16),
            pltpu.VMEM((S, D), bf16),
            pltpu.VMEM((6, S, D), bf16),
            pltpu.VMEM((6, S, D), bf16),
            pltpu.SemaphoreType.DMA((3,)),
            pltpu.SemaphoreType.DMA((13,)),
            pltpu.SemaphoreType.DMA((6,)),
            pltpu.SemaphoreType.DMA((6,)),
            pltpu.SemaphoreType.DMA((6,)),
            pltpu.SemaphoreType.DMA((6,)),
        ],
        compiler_params=pltpu.CompilerParams(collective_id=0, vmem_limit_bytes=100 * 1024 * 1024),
    )(x, Wq, Wk, Wv, Wo, jnp.asarray(_TABLES))
```

```python
import jax
import jax.numpy as jnp
import numpy as np
from jax import lax
from jax.experimental import pallas as pl
from jax.experimental.pallas import tpu as pltpu

N_DEV = 4
BL, S, D = 2, 512, 1024
HL, DH = 8, 128
SCALE = 0.08838834764831843
LOG2E = 1.4426950408889634


def _rope_tables():
    inv = 1.0 / (10000.0 ** (np.arange(0, DH, 2) / DH))
    pos = np.arange(S)[:, None] * inv[None, :]
    cos = np.repeat(np.cos(pos), 2, axis=-1).astype(np.float32)
    sin = np.repeat(np.sin(pos), 2, axis=-1).astype(np.float32)
    sign = np.where(np.arange(DH) % 2 == 0, -1.0, 1.0).astype(np.float32)
    sin = sin * sign[None, :]
    return np.stack([cos, sin]).astype(np.float32)


_TABLES = _rope_tables()


def pallas_dist_rope_attn_htp_bs_b2_sq512_d1024_hq8_dh128_kernel(x, Wq, Wk, Wv, Wo):
    f32, bf16 = jnp.float32, jnp.bfloat16
    MESH = pl.DeviceIdType.MESH

    def body(x_hbm, wq_hbm, wk_hbm, wv_hbm, wo_hbm, tab_hbm, out_ref,
             tab_ref,             xst, wst, ws, wo, xs, x_all, ctx, ctx0, sbuf, rbuf,
             x_sems, w_sems, ag_s, ag_r, rs_s, rs_r):
        me = lax.axis_index("i")
        right = lax.rem(me + 1, N_DEV)
        left = lax.rem(me + 3, N_DEV)
        diag = lax.rem(me + 2, N_DEV)

        NP = HL // 2
        PW = 2 * DH
        w_hbm = (wq_hbm, wk_hbm, wv_hbm)

        def x_ld(b):
            return pltpu.make_async_copy(x_hbm.at[b], xst.at[b], x_sems.at[b])

        def w_ld(i, hp):
            cols = pl.ds(hp * PW, PW)
            return pltpu.make_async_copy(w_hbm[i].at[:, cols], wst.at[i, :, cols],
                                         w_sems.at[i * NP + hp])

        wo_ld = pltpu.make_async_copy(wo_hbm, wst.at[3], w_sems.at[3 * NP])

        def ag(src_slot, dst_slot, dev):
            return pltpu.make_async_remote_copy(
                src_ref=x_all.at[src_slot], dst_ref=x_all.at[dst_slot],
                send_sem=ag_s.at[dst_slot - 1], recv_sem=ag_r.at[dst_slot - 1],
                device_id=(dev,), device_id_type=MESH)

        def rs(step, dev):
            return pltpu.make_async_remote_copy(
                src_ref=sbuf.at[step - 1], dst_ref=rbuf.at[step - 1],
                send_sem=rs_s.at[step - 1], recv_sem=rs_r.at[step - 1],
                device_id=(dev,), device_id_type=MESH)

        even = (lax.broadcasted_iota(jnp.int32, (S, DH), 1) % 2) == 0

        def rope(t, c, s):
            sw = jnp.where(even, pltpu.roll(t, DH - 1, 1), pltpu.roll(t, 1, 1))
            return (t * c + sw * s).astype(bf16)

        HS, HD = S // 2, D // 2

        def rhs_terms(b11, b12, b21, b22):
            return b11 + b22, b11, b12 - b22, b21 - b11, b22, b11 + b12, b21 + b22

        def out_proj(c, nxt=None):
            a11, a12, a21, a22 = c[:HS, :HD], c[:HS, HD:], c[HS:, :HD], c[HS:, HD:]
            m3 = jnp.dot(a11, wo[2], preferred_element_type=f32)
            m4 = jnp.dot(a22, wo[3], preferred_element_type=f32)
            f11, f12, f21, f22 = (t.astype(f32) for t in (a11, a12, a21, a22))
            lhs = ((f11 + f22).astype(bf16), (f21 + f22).astype(bf16), a11, a22,
                   (f11 + f12).astype(bf16), (f21 - f11).astype(bf16), (f12 - f22).astype(bf16))
            m1, m2 = (jnp.dot(lhs[n], wo[n], preferred_element_type=f32) for n in (0, 1))
            if nxt is not None:
                prep_x(nxt)
            m5, m6, m7 = (jnp.dot(lhs[n], wo[n], preferred_element_type=f32) for n in (4, 5, 6))
            return jnp.concatenate(
                [jnp.concatenate([(m1 + m4) + (m7 - m5), m3 + m5], axis=1),
                 jnp.concatenate([m2 + m4, (m1 - m2) + (m3 + m6)], axis=1)], axis=0)

        def prep_w(hp):
            for i in range(3):
                ld_wait(2 if (i == 2 and hp == 0) else 1)
                c0 = slice(hp * PW, hp * PW + DH)
                c1 = slice(hp * PW + DH, (hp + 1) * PW)
                b11, b12 = wst[i, :HD, c0], wst[i, :HD, c1]
                b21, b22 = wst[i, HD:, c0], wst[i, HD:, c1]
                if i == 0:
                    b11, b12, b21, b22 = (t * (SCALE * LOG2E) for t in (b11, b12, b21, b22))
                for n, t in enumerate(rhs_terms(b11, b12, b21, b22)):
                    ws[hp, n, :, i * DH:(i + 1) * DH] = t.astype(bf16)

        def prep_x(slot):
            a11 = x_all[slot, :HS, :HD].astype(f32)
            a12 = x_all[slot, :HS, HD:].astype(f32)
            a21 = x_all[slot, HS:, :HD].astype(f32)
            a22 = x_all[slot, HS:, HD:].astype(f32)
            for n, t in enumerate((a11 + a22, a21 + a22, a11 + a12, a21 - a11, a12 - a22)):
                xs[n] = t.astype(bf16)

        def attention(slot, ctx, first=False):
            if first:
                prep_w(0)
            for hp in range(NP):
                lhs = (xs[0], xs[1], x_all[slot, :HS, :HD], x_all[slot, HS:, HD:], xs[2], xs[3], xs[4])
                m1, m2, m3, m4, m5, m6, m7 = (
                    jnp.dot(lhs[n], ws[hp, n], preferred_element_type=f32) for n in range(7))
                heads = (jnp.concatenate([(m1 + m4) + (m7 - m5), m2 + m4], axis=0),
                         jnp.concatenate([m3 + m5, (m1 - m2) + (m3 + m6)], axis=0))
                qkv = [(rope(t[:, :DH], tab_ref[0], tab_ref[1]),
                        rope(t[:, DH:2 * DH], tab_ref[0], tab_ref[1]),
                        t[:, 2 * DH:].astype(bf16)) for t in heads]
                if first and hp + 1 < NP:
                    prep_w(hp + 1)
                for j in range(2):
                    h = hp * 2 + j
                    q, k, v = qkv[j]
                    sc = lax.dot_general(q, k, (((1,), (1,)), ((), ())),
                                         preferred_element_type=f32)
                    m = jnp.max(sc, axis=-1, keepdims=True)
                    p = jnp.exp2(sc - m)
                    l = jnp.sum(p, axis=-1, keepdims=True)
                    o = jnp.dot(p.astype(bf16), v, preferred_element_type=f32)
                    ctx[:, h * DH:(h + 1) * DH] = (o / l).astype(bf16)

        loads = [x_ld(0), w_ld(0, 0), w_ld(1, 0), w_ld(2, 0),
                 pltpu.make_async_copy(tab_hbm, tab_ref, x_sems.at[2])]
        loads += [w_ld(i, hp) for hp in (1, 2, 3) for i in range(3)] + [x_ld(1), wo_ld]
        pos = [0, 2]

        def ld_wait(n=1):
            for _ in range(n):
                loads[pos[0]].wait()
                pos[0] += 1
            while pos[1] < min(pos[0] + 4, len(loads)):
                loads[pos[1]].start()
                pos[1] += 1

        for c in loads[:2]:
            c.start()
        bar = pltpu.get_barrier_semaphore()
        for d in (left, right):
            pl.semaphore_signal(bar, inc=1, device_id=(d,), device_id_type=MESH)
        ld_wait()
        x_all[0] = xst[0].astype(bf16)
        pl.semaphore_wait(bar, 2)
        ag(0, 1, right).start()
        ag(0, 2, left).start()
        prep_x(0)
        attention(0, ctx0, first=True)
        ld_wait(2)
        x_all[7] = xst[1].astype(bf16)
        ag(7, 4, left).start()
        ag(0, 1, me).wait_recv()
        ag(1, 3, right).start()
        ag(0, 2, me).wait_recv()
        prep_x(1)
        for n, t in enumerate(rhs_terms(wst[3, :HD, :HD], wst[3, :HD, HD:],
                                        wst[3, HD:, :HD], wst[3, HD:, HD:])):
            wo[n] = t.astype(bf16)

        def step_fn(s, carry):
            attention(s, ctx)

            part = out_proj(ctx, s + 1)
            sbuf[s - 1] = part.astype(bf16)

            @pl.when(s == 6)
            def _():
                rs(5, me).wait_recv()
                sbuf[5] = (part + rbuf[4].astype(f32)).astype(bf16)

            @pl.when(s != 2)
            def _():
                rs(s, jnp.where(jnp.logical_or(s == 3, s == 4), right, left)).start()

            @pl.when(s == 4)
            def _():
                rs(3, me).wait_recv()
                sbuf[1] = (sbuf[1].astype(f32) + rbuf[2].astype(f32)).astype(bf16)
                rs(2, right).start()

            @pl.when(s == 1)
            def _():
                ag(7, 6, right).start()
                ag(0, 4, me).wait_recv()
                ag(4, 5, left).start()

            @pl.when(jnp.logical_and(s != 2, s <= 4))
            def _():
                ag(0, s + 2, me).wait_recv()

            return carry

        lax.fori_loop(1, 7, step_fn, 0)

        for t in (1, 2):
            rs(t, me).wait_recv()
        part = out_proj(ctx0)
        out_ref[0] = part + (rbuf[0].astype(f32) + rbuf[1].astype(f32))
        attention(7, ctx)
        for t in (4, 6):
            rs(t, me).wait_recv()
        part = out_proj(ctx)
        out_ref[1] = part + (rbuf[3].astype(f32) + rbuf[5].astype(f32))

        for t in range(1, 7):
            ag(0, t, me).wait_send()
            rs(t, me).wait_send()

    any_spec = pl.BlockSpec(memory_space=pl.ANY)
    return pl.pallas_call(
        body,
        out_shape=jax.ShapeDtypeStruct((BL, S, D), f32),
        in_specs=[any_spec] * 6,
        out_specs=pl.BlockSpec((BL, S, D), lambda: (0, 0, 0)),
        scratch_shapes=[
            pltpu.VMEM((2, S, DH), f32),
            pltpu.VMEM((BL, S, D), f32),
            pltpu.VMEM((4, D, D), f32),
            pltpu.VMEM((HL // 2, 7, D // 2, 3 * DH), bf16),
            pltpu.VMEM((7, D // 2, D // 2), bf16),
            pltpu.VMEM((5, S // 2, D // 2), bf16),
            pltpu.VMEM((8, S, D), bf16),
            pltpu.VMEM((S, D), bf16),
            pltpu.VMEM((S, D), bf16),
            pltpu.VMEM((6, S, D), bf16),
            pltpu.VMEM((6, S, D), bf16),
            pltpu.SemaphoreType.DMA((3,)),
            pltpu.SemaphoreType.DMA((13,)),
            pltpu.SemaphoreType.DMA((6,)),
            pltpu.SemaphoreType.DMA((6,)),
            pltpu.SemaphoreType.DMA((6,)),
            pltpu.SemaphoreType.DMA((6,)),
        ],
        compiler_params=pltpu.CompilerParams(collective_id=0, vmem_limit_bytes=100 * 1024 * 1024),
    )(x, Wq, Wk, Wv, Wo, jnp.asarray(_TABLES))
```

```python
import jax
import jax.numpy as jnp
import numpy as np
from jax import lax
from jax.experimental import pallas as pl
from jax.experimental.pallas import tpu as pltpu

N_DEV = 4
BL, S, D = 2, 512, 1024
HL, DH = 8, 128
SCALE = 0.08838834764831843
LOG2E = 1.4426950408889634


def _rope_tables():
    inv = 1.0 / (10000.0 ** (np.arange(0, DH, 2) / DH))
    pos = np.arange(S)[:, None] * inv[None, :]
    cos = np.repeat(np.cos(pos), 2, axis=-1).astype(np.float32)
    sin = np.repeat(np.sin(pos), 2, axis=-1).astype(np.float32)
    sign = np.where(np.arange(DH) % 2 == 0, -1.0, 1.0).astype(np.float32)
    sin = sin * sign[None, :]
    return np.stack([cos, sin]).astype(np.float32)


_TABLES = _rope_tables()


def pallas_dist_rope_attn_htp_bs_b2_sq512_d1024_hq8_dh128_kernel(x, Wq, Wk, Wv, Wo):
    f32, bf16 = jnp.float32, jnp.bfloat16
    MESH = pl.DeviceIdType.MESH

    def body(x_hbm, wq_hbm, wk_hbm, wv_hbm, wo_hbm, tab_hbm, out_ref,
             tab_ref,             xst, wst, wqk, ws, wo, xs, x_all, ctx, ctx0, sbuf, rbuf,
             x_sems, w_sems, ag_s, ag_r, rs_s, rs_r):
        me = lax.axis_index("i")
        right = lax.rem(me + 1, N_DEV)
        left = lax.rem(me + 3, N_DEV)
        diag = lax.rem(me + 2, N_DEV)

        NP = HL // 2
        PW = 2 * DH
        w_hbm = (wq_hbm, wk_hbm, wv_hbm)

        def x_ld(b):
            return pltpu.make_async_copy(x_hbm.at[b], xst.at[b], x_sems.at[b])

        def w_ld(i, hp):
            cols = pl.ds(hp * PW, PW)
            return pltpu.make_async_copy(w_hbm[i].at[:, cols], wst.at[i, :, cols],
                                         w_sems.at[i * NP + hp])

        wo_ld = pltpu.make_async_copy(wo_hbm, wst.at[3], w_sems.at[3 * NP])

        def ag(src_slot, dst_slot, dev):
            return pltpu.make_async_remote_copy(
                src_ref=x_all.at[src_slot], dst_ref=x_all.at[dst_slot],
                send_sem=ag_s.at[dst_slot - 1], recv_sem=ag_r.at[dst_slot - 1],
                device_id=(dev,), device_id_type=MESH)

        def rs(step, dev):
            return pltpu.make_async_remote_copy(
                src_ref=sbuf.at[step - 1], dst_ref=rbuf.at[step - 1],
                send_sem=rs_s.at[step - 1], recv_sem=rs_r.at[step - 1],
                device_id=(dev,), device_id_type=MESH)

        even = (lax.broadcasted_iota(jnp.int32, (S, DH), 1) % 2) == 0

        def rope(t, c, s):
            sw = jnp.where(even, pltpu.roll(t, DH - 1, 1), pltpu.roll(t, 1, 1))
            return (t * c + sw * s).astype(bf16)

        HS, HD = S // 2, D // 2

        def rhs_terms(b11, b12, b21, b22):
            return b11 + b22, b11, b12 - b22, b21 - b11, b22, b11 + b12, b21 + b22

        def out_proj(c, nxt=None):
            a11, a12, a21, a22 = c[:HS, :HD], c[:HS, HD:], c[HS:, :HD], c[HS:, HD:]
            m3 = jnp.dot(a11, wo[2], preferred_element_type=f32)
            m4 = jnp.dot(a22, wo[3], preferred_element_type=f32)
            f11, f12, f21, f22 = (t.astype(f32) for t in (a11, a12, a21, a22))
            lhs = ((f11 + f22).astype(bf16), (f21 + f22).astype(bf16), a11, a22,
                   (f11 + f12).astype(bf16), (f21 - f11).astype(bf16), (f12 - f22).astype(bf16))
            m1, m2 = (jnp.dot(lhs[n], wo[n], preferred_element_type=f32) for n in (0, 1))
            if nxt is not None:
                prep_x(nxt)
            m5, m6, m7 = (jnp.dot(lhs[n], wo[n], preferred_element_type=f32) for n in (4, 5, 6))
            return jnp.concatenate(
                [jnp.concatenate([(m1 + m4) + (m7 - m5), m3 + m5], axis=1),
                 jnp.concatenate([m2 + m4, (m1 - m2) + (m3 + m6)], axis=1)], axis=0)

        def prep_w(hp):
            for i in range(3):
                ld_wait(2 if (i == 2 and hp == 0) else 1)
                if i < 2:
                    w = wst[i, :, hp * PW:(hp + 1) * PW]
                    if i == 0:
                        w = w * (SCALE * LOG2E)
                    wqk[hp, :, i * PW:(i + 1) * PW] = w.astype(bf16)
                else:
                    c0 = slice(hp * PW, hp * PW + DH)
                    c1 = slice(hp * PW + DH, (hp + 1) * PW)
                    for n, t in enumerate(rhs_terms(wst[i, :HD, c0], wst[i, :HD, c1],
                                                    wst[i, HD:, c0], wst[i, HD:, c1])):
                        ws[hp, n] = t.astype(bf16)

        def prep_x(slot):
            a11 = x_all[slot, :HS, :HD].astype(f32)
            a12 = x_all[slot, :HS, HD:].astype(f32)
            a21 = x_all[slot, HS:, :HD].astype(f32)
            a22 = x_all[slot, HS:, HD:].astype(f32)
            for n, t in enumerate((a11 + a22, a21 + a22, a11 + a12, a21 - a11, a12 - a22)):
                xs[n] = t.astype(bf16)

        def attention(slot, ctx, first=False):
            if first:
                prep_w(0)
            for hp in range(NP):
                qk = jnp.dot(x_all[slot], wqk[hp], preferred_element_type=f32)
                lhs = (xs[0], xs[1], x_all[slot, :HS, :HD], x_all[slot, HS:, HD:], xs[2], xs[3], xs[4])
                m1, m2, m3, m4, m5, m6, m7 = (
                    jnp.dot(lhs[n], ws[hp, n], preferred_element_type=f32) for n in range(7))
                heads = (jnp.concatenate([(m1 + m4) + (m7 - m5), m2 + m4], axis=0),
                         jnp.concatenate([m3 + m5, (m1 - m2) + (m3 + m6)], axis=0))
                qkv = [(rope(qk[:, j * DH:(j + 1) * DH], tab_ref[0], tab_ref[1]),
                        rope(qk[:, PW + j * DH:PW + (j + 1) * DH], tab_ref[0], tab_ref[1]),
                        heads[j].astype(bf16)) for j in range(2)]
                if first and hp + 1 < NP:
                    prep_w(hp + 1)
                for j in range(2):
                    h = hp * 2 + j
                    q, k, v = qkv[j]
                    sc = lax.dot_general(q, k, (((1,), (1,)), ((), ())),
                                         preferred_element_type=f32)
                    m = jnp.max(sc, axis=-1, keepdims=True)
                    p = jnp.exp2(sc - m)
                    l = jnp.sum(p, axis=-1, keepdims=True)
                    o = jnp.dot(p.astype(bf16), v, preferred_element_type=f32)
                    ctx[:, h * DH:(h + 1) * DH] = (o / l).astype(bf16)

        loads = [x_ld(0), w_ld(0, 0), w_ld(1, 0), w_ld(2, 0),
                 pltpu.make_async_copy(tab_hbm, tab_ref, x_sems.at[2])]
        loads += [w_ld(i, hp) for hp in (1, 2, 3) for i in range(3)] + [x_ld(1), wo_ld]
        pos = [0, 2]

        def ld_wait(n=1):
            for _ in range(n):
                loads[pos[0]].wait()
                pos[0] += 1
            while pos[1] < min(pos[0] + 4, len(loads)):
                loads[pos[1]].start()
                pos[1] += 1

        for c in loads[:2]:
            c.start()
        bar = pltpu.get_barrier_semaphore()
        for d in (left, right):
            pl.semaphore_signal(bar, inc=1, device_id=(d,), device_id_type=MESH)
        ld_wait()
        x_all[0] = xst[0].astype(bf16)
        pl.semaphore_wait(bar, 2)
        ag(0, 1, right).start()
        ag(0, 2, left).start()
        prep_x(0)
        attention(0, ctx0, first=True)
        ld_wait(2)
        x_all[7] = xst[1].astype(bf16)
        ag(7, 4, left).start()
        ag(0, 1, me).wait_recv()
        ag(1, 3, right).start()
        ag(0, 2, me).wait_recv()
        prep_x(1)
        for n, t in enumerate(rhs_terms(wst[3, :HD, :HD], wst[3, :HD, HD:],
                                        wst[3, HD:, :HD], wst[3, HD:, HD:])):
            wo[n] = t.astype(bf16)

        def step_fn(s, carry):
            attention(s, ctx)

            part = out_proj(ctx, s + 1)
            sbuf[s - 1] = part.astype(bf16)

            @pl.when(s == 6)
            def _():
                rs(5, me).wait_recv()
                sbuf[5] = (part + rbuf[4].astype(f32)).astype(bf16)

            @pl.when(s != 2)
            def _():
                rs(s, jnp.where(jnp.logical_or(s == 3, s == 4), right, left)).start()

            @pl.when(s == 4)
            def _():
                rs(3, me).wait_recv()
                sbuf[1] = (sbuf[1].astype(f32) + rbuf[2].astype(f32)).astype(bf16)
                rs(2, right).start()

            @pl.when(s == 1)
            def _():
                ag(7, 6, right).start()
                ag(0, 4, me).wait_recv()
                ag(4, 5, left).start()

            @pl.when(jnp.logical_and(s != 2, s <= 4))
            def _():
                ag(0, s + 2, me).wait_recv()

            return carry

        lax.fori_loop(1, 7, step_fn, 0)

        for t in (1, 2):
            rs(t, me).wait_recv()
        part = out_proj(ctx0)
        out_ref[0] = part + (rbuf[0].astype(f32) + rbuf[1].astype(f32))
        attention(7, ctx)
        for t in (4, 6):
            rs(t, me).wait_recv()
        part = out_proj(ctx)
        out_ref[1] = part + (rbuf[3].astype(f32) + rbuf[5].astype(f32))

        for t in range(1, 7):
            ag(0, t, me).wait_send()
            rs(t, me).wait_send()

    any_spec = pl.BlockSpec(memory_space=pl.ANY)
    return pl.pallas_call(
        body,
        out_shape=jax.ShapeDtypeStruct((BL, S, D), f32),
        in_specs=[any_spec] * 6,
        out_specs=pl.BlockSpec((BL, S, D), lambda: (0, 0, 0)),
        scratch_shapes=[
            pltpu.VMEM((2, S, DH), f32),
            pltpu.VMEM((BL, S, D), f32),
            pltpu.VMEM((4, D, D), f32),
            pltpu.VMEM((HL // 2, D, 4 * DH), bf16),
            pltpu.VMEM((HL // 2, 7, D // 2, DH), bf16),
            pltpu.VMEM((7, D // 2, D // 2), bf16),
            pltpu.VMEM((5, S // 2, D // 2), bf16),
            pltpu.VMEM((8, S, D), bf16),
            pltpu.VMEM((S, D), bf16),
            pltpu.VMEM((S, D), bf16),
            pltpu.VMEM((6, S, D), bf16),
            pltpu.VMEM((6, S, D), bf16),
            pltpu.SemaphoreType.DMA((3,)),
            pltpu.SemaphoreType.DMA((13,)),
            pltpu.SemaphoreType.DMA((6,)),
            pltpu.SemaphoreType.DMA((6,)),
            pltpu.SemaphoreType.DMA((6,)),
            pltpu.SemaphoreType.DMA((6,)),
        ],
        compiler_params=pltpu.CompilerParams(collective_id=0, vmem_limit_bytes=100 * 1024 * 1024),
    )(x, Wq, Wk, Wv, Wo, jnp.asarray(_TABLES))
```
